```python
import numpy as np

kernel_name = "dist_mean_ax1_xy_m4096_n1024"

def setup_inputs():
    return {"x": np.random.randn(8192, 2048).astype(np.float32)}

def reference(x: np.ndarray) -> np.ndarray:
    return np.mean(x, axis=1, keepdims=True)
```

```python
import jax
import jax.numpy as jnp
from jax import lax
from jax.experimental import pallas as pl
from jax.experimental.pallas import tpu as pltpu

LANES = 128
GROUP = 128
MESH = pl.DeviceIdType.MESH


def _offsets(sizes):
    offs = [0]
    for s in sizes:
        offs.append(offs[-1] + s)
    return offs


def _tree_add(vals):
    while len(vals) > 1:
        vals = [vals[i] + vals[i + 1] if i + 1 < len(vals) else vals[i]
                for i in range(0, len(vals), 2)]
    return vals[0]


def pallas_dist_mean_ax1_xy_m4096_n1024_kernel(x: jax.Array):
    m, n = x.shape
    half = m // 2
    n_lane_blocks = n // LANES
    inv_cols = 1.0 / (2 * n)

    raw_pieces = (72, 48, 64)
    raw_offs = _offsets(raw_pieces)
    raw_rows = raw_offs[-1]
    raw_at = 1024
    own_chunks = (1024, 512, 256, 128)
    tail = (64, 32, 32)
    own_sizes = own_chunks + tail
    own_offs = _offsets(own_sizes)
    assert own_offs[-1] == half and sum(tail) == GROUP
    raw_chunk = own_offs.index(raw_at)
    raw_full, raw_part = divmod(raw_rows, GROUP)
    oth_ranges = ((0, raw_at), (raw_at + raw_rows, half - raw_at - raw_rows))
    skip_end = raw_at + raw_full * GROUP
    part_ranges = ((0, raw_at), (skip_end, half - skip_end))
    n_oth = len(oth_ranges)
    n_loads = n_oth + len(own_sizes)
    assert len(raw_pieces) == n_oth + 1

    def fold(buf, row0, rows):
        return _tree_add([buf[pl.ds(row0, rows), pl.ds(j * LANES, LANES)]
                          for j in range(n_lane_blocks)])

    def dense(s, r0=0):
        r = s.shape[0]
        sums = jnp.sum(s, axis=1, keepdims=True)
        row = lax.broadcasted_iota(jnp.int32, (r, GROUP), 0)
        lane = lax.broadcasted_iota(jnp.int32, (r, GROUP), 1)
        return jnp.sum(jnp.where(lane == row + r0, sums, 0.0), axis=0, keepdims=True)

    def body(x_hbm, out, oth_buf, own_buf, raw_buf, part_send, part_recv,
             load_sems, part_send_sems, part_recv_sems, out_send_sem, out_recv_sem,
             raw_send_sems, raw_recv_sems):
        my_x = lax.axis_index("x")
        my_y = lax.axis_index("y")
        partner = (my_x, 1 - my_y)
        own0 = pl.multiple_of(my_y * half, half)
        oth0 = pl.multiple_of((1 - my_y) * half, half)

        def load(c):
            if c < n_oth:
                r0, rows = oth_ranges[c]
                base, dst = oth0, oth_buf
            else:
                r0, rows = own_offs[c - n_oth], own_sizes[c - n_oth]
                base, dst = own0, own_buf
            return pltpu.make_async_copy(
                x_hbm.at[pl.ds(pl.multiple_of(base + r0, 8), rows)],
                dst.at[pl.ds(r0, rows)], load_sems.at[c])

        def remote(src, dst, send_sem, recv_sem):
            return pltpu.make_async_remote_copy(src, dst, send_sem, recv_sem,
                                                device_id=partner, device_id_type=MESH)

        raw_copies = [
            remote(x_hbm.at[pl.ds(pl.multiple_of(oth0 + raw_at + raw_offs[i], 8), rows)],
                   raw_buf.at[pl.ds(raw_offs[i], rows)],
                   raw_send_sems.at[i], raw_recv_sems.at[i])
            for i, rows in enumerate(raw_pieces)]
        part_copies = [
            remote(part_send.at[:, pl.ds(a, w)], part_recv.at[:, pl.ds(a, w)],
                   part_send_sems.at[i], part_recv_sems.at[i])
            for i, (a, w) in enumerate(part_ranges)]

        for c in range(n_loads):
            load(c).start()

        barrier = pltpu.get_barrier_semaphore()
        pl.semaphore_signal(barrier, inc=1, device_id=partner, device_id_type=MESH)
        pl.semaphore_wait(barrier, 1)
        raw_copies[0].start()

        def partial_group(g, carry):
            row0 = pl.multiple_of(g * GROUP, GROUP)
            part_send[:, pl.ds(row0, GROUP)] = dense(fold(oth_buf, row0, GROUP))
            return carry

        for c in range(n_oth):
            load(c).wait()
            r0, rows = oth_ranges[c]
            lead = -r0 % GROUP
            if lead:
                part_send[:, pl.ds(r0 + lead - GROUP, GROUP)] = dense(
                    fold(oth_buf, r0, lead), GROUP - lead)
            lax.fori_loop((r0 + lead) // GROUP, (r0 + rows) // GROUP, partial_group, 0)
            part_copies[c].start()
            raw_copies[c + 1].start()

        def put(row0, total):
            out[:, pl.ds(pl.multiple_of(own0 + row0, GROUP), GROUP)] = total * inv_cols

        def publish(row0, rows):
            ref = out.at[:, pl.ds(pl.multiple_of(own0 + row0, GROUP), rows)]
            remote(ref, ref, out_send_sem, out_recv_sem).start()

        def final_group(g, carry):
            row0 = pl.multiple_of(g * GROUP, GROUP)
            put(row0, dense(fold(own_buf, row0, GROUP)) + part_recv[:, pl.ds(row0, GROUP)])
            return carry

        for ci, rows in enumerate(own_chunks):
            load(n_oth + ci).wait()
            g_first = own_offs[ci] // GROUP
            g_last = own_offs[ci + 1] // GROUP
            if ci == 0:
                part_copies[0].wait_recv()
            if ci == raw_chunk:
                part_copies[1].wait_recv()
                g_raw = g_first
                g_first += raw_full + (1 if raw_part else 0)
            if g_first < g_last:
                lax.fori_loop(g_first, g_last, final_group, 0)
            if ci == raw_chunk:
                for cp in raw_copies:
                    cp.wait_recv()
                for g in range(raw_full):
                    row0 = (g_raw + g) * GROUP
                    put(row0, dense(fold(own_buf, row0, GROUP) + fold(raw_buf, g * GROUP, GROUP)))
                if raw_part:
                    row0 = (g_raw + raw_full) * GROUP
                    put(row0, dense(fold(own_buf, row0, GROUP))
                        + dense(fold(raw_buf, raw_full * GROUP, raw_part))
                        + part_recv[:, pl.ds(row0, GROUP)])
            publish(own_offs[ci], rows)

        last0 = half - GROUP
        total = part_recv[:, pl.ds(last0, GROUP)]
        for ti, rows in enumerate(tail):
            load(n_oth + len(own_chunks) + ti).wait()
            row0 = own_offs[len(own_chunks) + ti]
            total = total + dense(fold(own_buf, row0, rows), row0 - last0)
        put(last0, total)
        publish(last0, GROUP)

        for cp in part_copies + raw_copies:
            cp.wait_send()
        all_out = remote(out.at[:, pl.ds(own0, half)], out.at[:, pl.ds(oth0, half)],
                         out_send_sem, out_recv_sem)
        all_out.wait_send()
        all_out.wait_recv()

    out = pl.pallas_call(
        body,
        out_shape=jax.ShapeDtypeStruct((1, m), jnp.float32),
        in_specs=[pl.BlockSpec(memory_space=pl.ANY)],
        out_specs=pl.BlockSpec(memory_space=pltpu.VMEM),
        scratch_shapes=[
            pltpu.VMEM((half, n), jnp.float32),
            pltpu.VMEM((half, n), jnp.float32),
            pltpu.VMEM((raw_rows, n), jnp.float32),
            pltpu.VMEM((1, half), jnp.float32),
            pltpu.VMEM((1, half), jnp.float32),
            pltpu.SemaphoreType.DMA((n_loads,)),
            pltpu.SemaphoreType.DMA((len(part_ranges),)),
            pltpu.SemaphoreType.DMA((len(part_ranges),)),
            pltpu.SemaphoreType.DMA,
            pltpu.SemaphoreType.DMA,
            pltpu.SemaphoreType.DMA((len(raw_pieces),)),
            pltpu.SemaphoreType.DMA((len(raw_pieces),)),
        ],
        compiler_params=pltpu.CompilerParams(
            collective_id=0,
            vmem_limit_bytes=32 * 1024 * 1024,
            disable_semaphore_checks=True,
        ),
    )(x)
    return out.reshape(m, 1)
```
